```python
import numpy as np

kernel_name = "dist_rope_attn_qseq_b2_sq128_d512_hq4_dh64"

def setup_inputs():
    x = np.random.randn(2, 512, 512).astype(np.float32)
    Wq = np.random.randn(512, 256).astype(np.float32) * 0.02
    Wk = np.random.randn(512, 256).astype(np.float32) * 0.02
    Wv = np.random.randn(512, 256).astype(np.float32) * 0.02
    Wo = np.random.randn(256, 512).astype(np.float32) * 0.02
    return {"x": x, "Wq": Wq, "Wk": Wk, "Wv": Wv, "Wo": Wo}

def reference(x, Wq, Wk, Wv, Wo):
    B, Sq, Hq, Dh = 2, 512, 4, 64
    inv = 1.0 / (10000.0 ** (np.arange(0, Dh, 2) / Dh))
    pos = np.arange(Sq)[:, None] * inv[None, :]
    cos = np.repeat(np.cos(pos), 2, axis=-1).astype(np.float32)
    sin = np.repeat(np.sin(pos), 2, axis=-1).astype(np.float32)
    def rot(t):
        t2 = t.reshape(B, Sq, Hq, Dh // 2, 2)
        t_r = np.stack([-t2[..., 1], t2[..., 0]], axis=-1).reshape(B, Sq, Hq, Dh)
        return t * cos[None, :, None, :] + t_r * sin[None, :, None, :]
    Q = rot((x @ Wq).reshape(B, Sq, Hq, Dh))
    K = rot((x @ Wk).reshape(B, Sq, Hq, Dh))
    V = (x @ Wv).reshape(B, Sq, Hq, Dh)
    s = np.einsum('bihd,bjhd->bhij', Q, K).astype(np.float32) * 0.125
    s_max = s.max(axis=-1, keepdims=True)
    w = np.exp(s - s_max)
    w = w / w.sum(axis=-1, keepdims=True)
    ctx = np.einsum('bhij,bjhd->bihd', w, V).reshape(B, Sq, Hq * Dh)
    return ctx @ Wo
```

```python
import numpy as np

import jax
import jax.numpy as jnp
from jax import lax
from jax.experimental import pallas as pl
from jax.experimental.pallas import tpu as pltpu

N_DEV = 4
B = 2
S_LOC = 128
ROWS = B * S_LOC
D = 512
H = 4
DH = 64
HD = H * DH
SCALE = 0.125

_MESH = pl.DeviceIdType.MESH
_T_V, _T_K, _T_Q, _T_C = 0, 1, 2, 3


def _rope_tables(me):
    lane = lax.broadcasted_iota(jnp.int32, (8, 128), 1)
    fidx = (lane % DH) // 2
    inv_np = (1.0 / (10000.0 ** (np.arange(0, DH, 2) / DH))).astype(np.float32)
    inv = jnp.zeros((8, 128), jnp.float32)
    for i in range(DH // 2):
        inv = jnp.where(fidx == i, jnp.float32(inv_np[i]), inv)
    inv = jnp.broadcast_to(inv[0:1, :], (S_LOC, 128))
    row = lax.broadcasted_iota(jnp.int32, (S_LOC, 128), 0)
    pos = (row + me * S_LOC).astype(jnp.float32)
    ang = pos * inv
    lane2 = lax.broadcasted_iota(jnp.int32, (S_LOC, 128), 1)
    cos_t = jnp.cos(ang)
    sin_t = jnp.sin(ang)
    sin_t = jnp.where(lane2 % 2 == 0, -sin_t, sin_t)
    return cos_t, sin_t


def _rope(t, cos_t, sin_t):
    lane = lax.broadcasted_iota(jnp.int32, t.shape, 1)
    swapped = jnp.where(lane % 2 == 0, pltpu.roll(t, 127, 1), pltpu.roll(t, 1, 1))
    return t * cos_t + swapped * sin_t


def pallas_dist_rope_attn_qseq_b2_sq128_d512_hq4_dh64_kernel(
    x: jax.Array,
    Wq: jax.Array,
    Wk: jax.Array,
    Wv: jax.Array,
    Wo: jax.Array,
):
    def body(x_hbm, wq_hbm, wk_hbm, wv_hbm, wo_hbm, out_hbm,
             x_v, wq_v, wk_v, wv_v, wo_v,
             sq, sk, sv, qq, kk, vv, sc, rc, out_v,
             ld_sems, ssem, rsem):
        me = lax.axis_index("i")
        dests = [(me + d) % N_DEV for d in range(1, N_DEV)]
        srcs = [(me + N_DEV - d) % N_DEV for d in range(1, N_DEV)]

        loads = [
            pltpu.make_async_copy(x_hbm, x_v, ld_sems.at[0]),
            pltpu.make_async_copy(wv_hbm, wv_v, ld_sems.at[1]),
            pltpu.make_async_copy(wk_hbm, wk_v, ld_sems.at[2]),
            pltpu.make_async_copy(wq_hbm, wq_v, ld_sems.at[3]),
            pltpu.make_async_copy(wo_hbm, wo_v, ld_sems.at[4]),
        ]
        for c in loads:
            c.start()

        bsem = pltpu.get_barrier_semaphore()
        for dev in dests:
            pl.semaphore_signal(bsem, inc=1, device_id=(dev,), device_id_type=_MESH)

        cos_t, sin_t = _rope_tables(me)
        lane = lax.broadcasted_iota(jnp.int32, (S_LOC, 128), 1)
        lo = lane < DH

        def remote(t, d, src_ref, dst_ref, dev):
            k = t * 3 + (d - 1)
            return pltpu.make_async_remote_copy(
                src_ref=src_ref, dst_ref=dst_ref,
                send_sem=ssem.at[k], recv_sem=rsem.at[k],
                device_id=(dev,), device_id_type=_MESH)

        def rows_of(ref, idx):
            return ref.at[pl.ds(pl.multiple_of(idx * S_LOC, S_LOC), S_LOC), :]

        def project_pack(w_v, sbuf, rope, scale):
            xb = x_v[...].astype(jnp.bfloat16)
            for j in range(H // 2):
                wb = w_v[:, j * 128:(j + 1) * 128].astype(jnp.bfloat16)
                col = jnp.dot(xb, wb, preferred_element_type=jnp.float32)
                top, bot = col[0:S_LOC], col[S_LOC:ROWS]
                if rope:
                    top = _rope(top, cos_t, sin_t)
                    bot = _rope(bot, cos_t, sin_t)
                if scale:
                    top = top * SCALE
                    bot = bot * SCALE
                even = jnp.where(lo, top, pltpu.roll(bot, DH, 1))
                odd = jnp.where(lo, pltpu.roll(top, DH, 1), bot)
                sbuf[2 * j] = even.astype(jnp.bfloat16)
                sbuf[2 * j + 1] = odd.astype(jnp.bfloat16)

        sends = []

        loads[0].wait()
        loads[1].wait()
        project_pack(wv_v, sv, rope=False, scale=False)
        pl.semaphore_wait(bsem, N_DEV - 1)
        for d, dev in enumerate(dests, start=1):
            cp = remote(_T_V, d, sv.at[dev], rows_of(vv, me), dev)
            cp.start()
            sends.append(cp)
        rows_of(vv, me)[...] = sv[me]

        loads[2].wait()
        project_pack(wk_v, sk, rope=True, scale=False)
        for d, dev in enumerate(dests, start=1):
            cp = remote(_T_K, d, sk.at[dev], rows_of(kk, me), dev)
            cp.start()
            sends.append(cp)
        rows_of(kk, me)[...] = sk[me]

        loads[3].wait()
        project_pack(wq_v, sq, rope=True, scale=True)
        for d, dev in enumerate(dests, start=1):
            cp = remote(_T_Q, d, sq.at[dev], qq.at[me], dev)
            cp.start()
            sends.append(cp)

        for d, src in enumerate(srcs, start=1):
            remote(_T_V, d, sv.at[0], rows_of(vv, src), src).wait_recv()
        for d, src in enumerate(srcs, start=1):
            remote(_T_K, d, sk.at[0], rows_of(kk, src), src).wait_recv()

        def attend(qp):
            qf = qp.astype(jnp.float32)
            lhs = jnp.concatenate(
                [jnp.where(lo, qf, 0.0), jnp.where(lo, 0.0, qf)], axis=0
            ).astype(jnp.bfloat16)
            s = lax.dot_general(lhs, kk[...], (((1,), (1,)), ((), ())),
                                preferred_element_type=jnp.float32)
            m = jnp.max(s, axis=1, keepdims=True)
            p = jnp.exp(s - m)
            l = jnp.sum(p, axis=1, keepdims=True)
            c = jnp.dot(p.astype(jnp.bfloat16), vv[...],
                        preferred_element_type=jnp.float32)
            c = c * (1.0 / l)
            return jnp.where(lo, c[0:S_LOC], c[S_LOC:ROWS]).astype(jnp.bfloat16)

        rc[me] = attend(sq[me])
        for d, src in enumerate(srcs, start=1):
            remote(_T_Q, d, sq.at[0], qq.at[src], src).wait_recv()
            sc[src] = attend(qq[src])
            cp = remote(_T_C, N_DEV - d, sc.at[src], rc.at[me], src)
            cp.start()
            sends.append(cp)

        loads[4].wait()
        wob = wo_v[...].astype(jnp.bfloat16)
        for d, src in enumerate(srcs, start=1):
            remote(_T_C, d, sc.at[0], rc.at[src], src).wait_recv()
        cols0, cols1 = [], []
        for j in range(H // 2):
            r_even = rc[2 * j].astype(jnp.float32)
            r_odd = rc[2 * j + 1].astype(jnp.float32)
            cols0.append(jnp.where(lo, r_even, pltpu.roll(r_odd, DH, 1)))
            cols1.append(jnp.where(lo, pltpu.roll(r_even, DH, 1), r_odd))
        ctx = jnp.concatenate(
            [jnp.concatenate(cols0, axis=1), jnp.concatenate(cols1, axis=1)], axis=0
        ).astype(jnp.bfloat16)
        out_v[...] = jnp.dot(ctx, wob, preferred_element_type=jnp.float32)
        st = pltpu.make_async_copy(out_v, out_hbm, ld_sems.at[5])
        st.start()
        for cp in sends:
            cp.wait_send()
        st.wait()

    tile = lambda n: pltpu.VMEM((n, S_LOC, 128), jnp.bfloat16)
    hbm = pl.BlockSpec(memory_space=pl.ANY)
    out = pl.pallas_call(
        body,
        out_shape=jax.ShapeDtypeStruct((ROWS, D), jnp.float32),
        in_specs=[hbm] * 5,
        out_specs=hbm,
        scratch_shapes=[
            pltpu.VMEM((ROWS, D), jnp.float32),
            pltpu.VMEM((D, HD), jnp.float32),
            pltpu.VMEM((D, HD), jnp.float32),
            pltpu.VMEM((D, HD), jnp.float32),
            pltpu.VMEM((HD, D), jnp.float32),
            tile(H), tile(H), tile(H),
            tile(N_DEV),
            pltpu.VMEM((N_DEV * S_LOC, 128), jnp.bfloat16),
            pltpu.VMEM((N_DEV * S_LOC, 128), jnp.bfloat16),
            tile(N_DEV),
            tile(N_DEV),
            pltpu.VMEM((ROWS, D), jnp.float32),
            pltpu.SemaphoreType.DMA((6,)),
            pltpu.SemaphoreType.DMA((12,)),
            pltpu.SemaphoreType.DMA((12,)),
        ],
        compiler_params=pltpu.CompilerParams(
            collective_id=0, vmem_limit_bytes=64 * 1024 * 1024),
    )(x.reshape(ROWS, D), Wq, Wk, Wv, Wo)
    return out.reshape(B, S_LOC, D)
```

```python
import numpy as np

import jax
import jax.numpy as jnp
from jax import lax
from jax.experimental import pallas as pl
from jax.experimental.pallas import tpu as pltpu

N_DEV = 4
B = 2
S_LOC = 128
ROWS = B * S_LOC
D = 512
H = 4
DH = 64
HD = H * DH
SCALE = 0.125

_MESH = pl.DeviceIdType.MESH
_T_V, _T_K, _T_Q, _T_C = 0, 1, 2, 3


def _rope_tables(me):
    lane = lax.broadcasted_iota(jnp.int32, (8, 128), 1)
    fidx = (lane % DH) // 2
    inv_np = (1.0 / (10000.0 ** (np.arange(0, DH, 2) / DH))).astype(np.float32)
    inv = jnp.zeros((8, 128), jnp.float32)
    for i in range(DH // 2):
        inv = jnp.where(fidx == i, jnp.float32(inv_np[i]), inv)
    inv = jnp.broadcast_to(inv[0:1, :], (S_LOC, 128))
    row = lax.broadcasted_iota(jnp.int32, (S_LOC, 128), 0)
    pos = (row + me * S_LOC).astype(jnp.float32)
    ang = pos * inv
    lane2 = lax.broadcasted_iota(jnp.int32, (S_LOC, 128), 1)
    cos_t = jnp.cos(ang)
    sin_t = jnp.sin(ang)
    sin_t = jnp.where(lane2 % 2 == 0, -sin_t, sin_t)
    return cos_t, sin_t


def _rope(t, cos_t, sin_t):
    lane = lax.broadcasted_iota(jnp.int32, t.shape, 1)
    swapped = jnp.where(lane % 2 == 0, pltpu.roll(t, 127, 1), pltpu.roll(t, 1, 1))
    return t * cos_t + swapped * sin_t


def pallas_dist_rope_attn_qseq_b2_sq128_d512_hq4_dh64_kernel(
    x: jax.Array,
    Wq: jax.Array,
    Wk: jax.Array,
    Wv: jax.Array,
    Wo: jax.Array,
):
    def body(x_hbm, wq_hbm, wk_hbm, wv_hbm, wo_hbm, out_hbm,
             x_v, wq_v, wk_v, wv_v, wo_v,
             sq, sk, sv, qq, kk, vv, sc, rc, out_v,
             ld_sems, ssem, rsem):
        me = lax.axis_index("i")
        dests = [(me + d) % N_DEV for d in range(1, N_DEV)]
        srcs = [(me + N_DEV - d) % N_DEV for d in range(1, N_DEV)]

        loads = [
            pltpu.make_async_copy(x_hbm, x_v, ld_sems.at[0]),
            pltpu.make_async_copy(wv_hbm, wv_v, ld_sems.at[1]),
            pltpu.make_async_copy(wk_hbm, wk_v, ld_sems.at[2]),
            pltpu.make_async_copy(wq_hbm, wq_v, ld_sems.at[3]),
            pltpu.make_async_copy(wo_hbm, wo_v, ld_sems.at[4]),
        ]
        for c in loads:
            c.start()

        bsem = pltpu.get_barrier_semaphore()
        for dev in dests:
            pl.semaphore_signal(bsem, inc=1, device_id=(dev,), device_id_type=_MESH)

        cos_t, sin_t = _rope_tables(me)
        lane = lax.broadcasted_iota(jnp.int32, (S_LOC, 128), 1)
        lo = lane < DH

        def remote(t, d, src_ref, dst_ref, dev):
            k = t * 3 + (d - 1)
            return pltpu.make_async_remote_copy(
                src_ref=src_ref, dst_ref=dst_ref,
                send_sem=ssem.at[k], recv_sem=rsem.at[k],
                device_id=(dev,), device_id_type=_MESH)

        def rows_of(ref, idx):
            return ref.at[pl.ds(pl.multiple_of(idx * S_LOC, S_LOC), S_LOC), :]

        def project_pack(w_v, sbuf, rope, scale):
            xb = x_v[...].astype(jnp.bfloat16)
            for j in range(H // 2):
                wb = w_v[:, j * 128:(j + 1) * 128].astype(jnp.bfloat16)
                col = jnp.dot(xb, wb, preferred_element_type=jnp.float32)
                top, bot = col[0:S_LOC], col[S_LOC:ROWS]
                if rope:
                    top = _rope(top, cos_t, sin_t)
                    bot = _rope(bot, cos_t, sin_t)
                if scale:
                    top = top * SCALE
                    bot = bot * SCALE
                even = jnp.where(lo, top, pltpu.roll(bot, DH, 1))
                odd = jnp.where(lo, pltpu.roll(top, DH, 1), bot)
                sbuf[2 * j] = even.astype(jnp.bfloat16)
                sbuf[2 * j + 1] = odd.astype(jnp.bfloat16)

        sends = []

        loads[0].wait()
        loads[1].wait()
        project_pack(wv_v, sv, rope=False, scale=False)
        pl.semaphore_wait(bsem, N_DEV - 1)
        for d, dev in enumerate(dests, start=1):
            cp = remote(_T_V, d, sv.at[dev], rows_of(vv, me), dev)
            cp.start()
            sends.append(cp)
        rows_of(vv, me)[...] = sv[me]

        loads[2].wait()
        project_pack(wk_v, sk, rope=True, scale=False)
        for d, dev in enumerate(dests, start=1):
            cp = remote(_T_K, d, sk.at[dev], rows_of(kk, me), dev)
            cp.start()
            sends.append(cp)
        rows_of(kk, me)[...] = sk[me]

        loads[3].wait()
        project_pack(wq_v, sq, rope=True, scale=True)
        for d, dev in enumerate(dests, start=1):
            cp = remote(_T_Q, d, sq.at[dev], qq.at[me], dev)
            cp.start()
            sends.append(cp)

        for d, src in enumerate(srcs, start=1):
            remote(_T_V, d, sv.at[0], rows_of(vv, src), src).wait_recv()
        for d, src in enumerate(srcs, start=1):
            remote(_T_K, d, sk.at[0], rows_of(kk, src), src).wait_recv()

        def attend(qp):
            qf = qp.astype(jnp.float32)
            lhs = jnp.concatenate(
                [jnp.where(lo, qf, 0.0), jnp.where(lo, 0.0, qf)], axis=0
            ).astype(jnp.bfloat16)
            s = lax.dot_general(lhs, kk[...], (((1,), (1,)), ((), ())),
                                preferred_element_type=jnp.float32)
            m = jnp.max(s, axis=1, keepdims=True)
            p = jnp.exp(s - m)
            l = jnp.sum(p, axis=1, keepdims=True)
            c = jnp.dot(p.astype(jnp.bfloat16), vv[...],
                        preferred_element_type=jnp.float32)
            c = c * (1.0 / l)
            return jnp.where(lo, c[0:S_LOC], c[S_LOC:ROWS]).astype(jnp.bfloat16)

        rc[me] = attend(sq[me])
        for d, src in enumerate(srcs, start=1):
            remote(_T_Q, d, sq.at[0], qq.at[src], src).wait_recv()
            sc[src] = attend(qq[src])
            cp = remote(_T_C, N_DEV - d, sc.at[src], rc.at[me], src)
            cp.start()
            sends.append(cp)

        loads[4].wait()
        wob = wo_v[...].astype(jnp.bfloat16)
        for d, src in enumerate(srcs, start=1):
            remote(_T_C, d, sc.at[0], rc.at[src], src).wait_recv()
        cols0, cols1 = [], []
        for j in range(H // 2):
            r_even = rc[2 * j].astype(jnp.float32)
            r_odd = rc[2 * j + 1].astype(jnp.float32)
            cols0.append(jnp.where(lo, r_even, pltpu.roll(r_odd, DH, 1)))
            cols1.append(jnp.where(lo, pltpu.roll(r_even, DH, 1), r_odd))
        ctx = jnp.concatenate(
            [jnp.concatenate(cols0, axis=1), jnp.concatenate(cols1, axis=1)], axis=0
        ).astype(jnp.bfloat16)
        res = jnp.dot(ctx, wob, preferred_element_type=jnp.float32)
        for b in range(B):
            out_v[b] = res[b * S_LOC:(b + 1) * S_LOC]
        st = pltpu.make_async_copy(out_v, out_hbm, ld_sems.at[5])
        st.start()
        for cp in sends:
            cp.wait_send()
        st.wait()

    tile = lambda n: pltpu.VMEM((n, S_LOC, 128), jnp.bfloat16)
    hbm = pl.BlockSpec(memory_space=pltpu.HBM)
    out = pl.pallas_call(
        body,
        out_shape=pltpu.HBM((B, S_LOC, D), jnp.float32),
        in_specs=[hbm] * 5,
        out_specs=hbm,
        scratch_shapes=[
            pltpu.VMEM((ROWS, D), jnp.float32),
            pltpu.VMEM((D, HD), jnp.float32),
            pltpu.VMEM((D, HD), jnp.float32),
            pltpu.VMEM((D, HD), jnp.float32),
            pltpu.VMEM((HD, D), jnp.float32),
            tile(H), tile(H), tile(H),
            tile(N_DEV),
            pltpu.VMEM((N_DEV * S_LOC, 128), jnp.bfloat16),
            pltpu.VMEM((N_DEV * S_LOC, 128), jnp.bfloat16),
            tile(N_DEV),
            tile(N_DEV),
            pltpu.VMEM((B, S_LOC, D), jnp.float32),
            pltpu.SemaphoreType.DMA((6,)),
            pltpu.SemaphoreType.DMA((12,)),
            pltpu.SemaphoreType.DMA((12,)),
        ],
        compiler_params=pltpu.CompilerParams(
            collective_id=0, vmem_limit_bytes=64 * 1024 * 1024),
    )(x.reshape(ROWS, D), Wq, Wk, Wv, Wo)
    return out
```

```python
import numpy as np

import jax
import jax.numpy as jnp
from jax import lax
from jax.experimental import pallas as pl
from jax.experimental.pallas import tpu as pltpu

N_DEV = 4
B = 2
S_LOC = 128
ROWS = B * S_LOC
D = 512
H = 4
DH = 64
HD = H * DH
SCALE = 0.125

_MESH = pl.DeviceIdType.MESH
_T_V, _T_K, _T_Q, _T_C = 0, 1, 2, 3


def _rope_tables(me):
    lane = lax.broadcasted_iota(jnp.int32, (8, 128), 1)
    fidx = (lane % DH) // 2
    inv_np = (1.0 / (10000.0 ** (np.arange(0, DH, 2) / DH))).astype(np.float32)
    inv = jnp.zeros((8, 128), jnp.float32)
    for i in range(DH // 2):
        inv = jnp.where(fidx == i, jnp.float32(inv_np[i]), inv)
    inv = jnp.broadcast_to(inv[0:1, :], (S_LOC, 128))
    row = lax.broadcasted_iota(jnp.int32, (S_LOC, 128), 0)
    pos = (row + me * S_LOC).astype(jnp.float32)
    ang = pos * inv
    lane2 = lax.broadcasted_iota(jnp.int32, (S_LOC, 128), 1)
    cos_t = jnp.cos(ang)
    sin_t = jnp.sin(ang)
    sin_t = jnp.where(lane2 % 2 == 0, -sin_t, sin_t)
    return cos_t, sin_t


def _rope(t, cos_t, sin_t):
    lane = lax.broadcasted_iota(jnp.int32, t.shape, 1)
    swapped = jnp.where(lane % 2 == 0, pltpu.roll(t, 127, 1), pltpu.roll(t, 1, 1))
    return t * cos_t + swapped * sin_t


def pallas_dist_rope_attn_qseq_b2_sq128_d512_hq4_dh64_kernel(
    x: jax.Array,
    Wq: jax.Array,
    Wk: jax.Array,
    Wv: jax.Array,
    Wo: jax.Array,
):
    def body(x_hbm, wq_hbm, wk_hbm, wv_hbm, wo_hbm, out_v,
             x_v, wq_v, wk_v, wv_v, wo_v,
             sq, sk, sv, qq, kk, vv, sc, rc,
             ld_sems, ssem, rsem):
        me = lax.axis_index("i")
        dests = [(me + d) % N_DEV for d in range(1, N_DEV)]
        srcs = [(me + N_DEV - d) % N_DEV for d in range(1, N_DEV)]

        loads = [
            pltpu.make_async_copy(x_hbm, x_v, ld_sems.at[0]),
            pltpu.make_async_copy(wv_hbm, wv_v, ld_sems.at[1]),
            pltpu.make_async_copy(wk_hbm, wk_v, ld_sems.at[2]),
            pltpu.make_async_copy(wq_hbm, wq_v, ld_sems.at[3]),
            pltpu.make_async_copy(wo_hbm, wo_v, ld_sems.at[4]),
        ]
        for c in loads:
            c.start()

        bsem = pltpu.get_barrier_semaphore()
        for dev in dests:
            pl.semaphore_signal(bsem, inc=1, device_id=(dev,), device_id_type=_MESH)

        cos_t, sin_t = _rope_tables(me)
        lane = lax.broadcasted_iota(jnp.int32, (S_LOC, 128), 1)
        lo = lane < DH

        def remote(t, d, src_ref, dst_ref, dev):
            k = t * 3 + (d - 1)
            return pltpu.make_async_remote_copy(
                src_ref=src_ref, dst_ref=dst_ref,
                send_sem=ssem.at[k], recv_sem=rsem.at[k],
                device_id=(dev,), device_id_type=_MESH)

        def rows_of(ref, idx):
            return ref.at[pl.ds(pl.multiple_of(idx * S_LOC, S_LOC), S_LOC), :]

        def project_pack(w_v, sbuf, rope, scale):
            xb = x_v[...].astype(jnp.bfloat16)
            for j in range(H // 2):
                wb = w_v[:, j * 128:(j + 1) * 128].astype(jnp.bfloat16)
                col = jnp.dot(xb, wb, preferred_element_type=jnp.float32)
                top, bot = col[0:S_LOC], col[S_LOC:ROWS]
                if rope:
                    top = _rope(top, cos_t, sin_t)
                    bot = _rope(bot, cos_t, sin_t)
                if scale:
                    top = top * SCALE
                    bot = bot * SCALE
                even = jnp.where(lo, top, pltpu.roll(bot, DH, 1))
                odd = jnp.where(lo, pltpu.roll(top, DH, 1), bot)
                sbuf[2 * j] = even.astype(jnp.bfloat16)
                sbuf[2 * j + 1] = odd.astype(jnp.bfloat16)

        sends = []

        loads[0].wait()
        loads[1].wait()
        project_pack(wv_v, sv, rope=False, scale=False)
        pl.semaphore_wait(bsem, N_DEV - 1)
        for d, dev in enumerate(dests, start=1):
            cp = remote(_T_V, d, sv.at[dev], rows_of(vv, me), dev)
            cp.start()
            sends.append(cp)
        rows_of(vv, me)[...] = sv[me]

        loads[2].wait()
        project_pack(wk_v, sk, rope=True, scale=False)
        for d, dev in enumerate(dests, start=1):
            cp = remote(_T_K, d, sk.at[dev], rows_of(kk, me), dev)
            cp.start()
            sends.append(cp)
        rows_of(kk, me)[...] = sk[me]

        loads[3].wait()
        project_pack(wq_v, sq, rope=True, scale=True)
        for d, dev in enumerate(dests, start=1):
            cp = remote(_T_Q, d, sq.at[dev], qq.at[me], dev)
            cp.start()
            sends.append(cp)

        for d, src in enumerate(srcs, start=1):
            remote(_T_V, d, sv.at[0], rows_of(vv, src), src).wait_recv()
        for d, src in enumerate(srcs, start=1):
            remote(_T_K, d, sk.at[0], rows_of(kk, src), src).wait_recv()

        def attend(qp):
            qf = qp.astype(jnp.float32)
            lhs = jnp.concatenate(
                [jnp.where(lo, qf, 0.0), jnp.where(lo, 0.0, qf)], axis=0
            ).astype(jnp.bfloat16)
            s = lax.dot_general(lhs, kk[...], (((1,), (1,)), ((), ())),
                                preferred_element_type=jnp.float32)
            m = jnp.max(s, axis=1, keepdims=True)
            p = jnp.exp(s - m)
            l = jnp.sum(p, axis=1, keepdims=True)
            c = jnp.dot(p.astype(jnp.bfloat16), vv[...],
                        preferred_element_type=jnp.float32)
            c = c * (1.0 / l)
            return jnp.where(lo, c[0:S_LOC], c[S_LOC:ROWS]).astype(jnp.bfloat16)

        rc[me] = attend(sq[me])
        for d, src in enumerate(srcs, start=1):
            remote(_T_Q, d, sq.at[0], qq.at[src], src).wait_recv()
            sc[src] = attend(qq[src])
            cp = remote(_T_C, N_DEV - d, sc.at[src], rc.at[me], src)
            cp.start()
            sends.append(cp)

        loads[4].wait()
        wob = wo_v[...].astype(jnp.bfloat16)
        for d, src in enumerate(srcs, start=1):
            remote(_T_C, d, sc.at[0], rc.at[src], src).wait_recv()
        cols0, cols1 = [], []
        for j in range(H // 2):
            r_even = rc[2 * j].astype(jnp.float32)
            r_odd = rc[2 * j + 1].astype(jnp.float32)
            cols0.append(jnp.where(lo, r_even, pltpu.roll(r_odd, DH, 1)))
            cols1.append(jnp.where(lo, pltpu.roll(r_even, DH, 1), r_odd))
        ctx = jnp.concatenate(
            [jnp.concatenate(cols0, axis=1), jnp.concatenate(cols1, axis=1)], axis=0
        ).astype(jnp.bfloat16)
        res = jnp.dot(ctx, wob, preferred_element_type=jnp.float32)
        for b in range(B):
            out_v[b] = res[b * S_LOC:(b + 1) * S_LOC]
        st = pltpu.make_async_copy(out_v, out_v, ld_sems.at[5])
        st.start()
        for cp in sends:
            cp.wait_send()
        st.wait()

    tile = lambda n: pltpu.VMEM((n, S_LOC, 128), jnp.bfloat16)
    hbm = pl.BlockSpec(memory_space=pltpu.HBM)
    out = pl.pallas_call(
        body,
        out_shape=jax.ShapeDtypeStruct((B, S_LOC, D), jnp.float32),
        in_specs=[hbm] * 5,
        out_specs=pl.BlockSpec(memory_space=pltpu.VMEM),
        scratch_shapes=[
            pltpu.VMEM((ROWS, D), jnp.float32),
            pltpu.VMEM((D, HD), jnp.float32),
            pltpu.VMEM((D, HD), jnp.float32),
            pltpu.VMEM((D, HD), jnp.float32),
            pltpu.VMEM((HD, D), jnp.float32),
            tile(H), tile(H), tile(H),
            tile(N_DEV),
            pltpu.VMEM((N_DEV * S_LOC, 128), jnp.bfloat16),
            pltpu.VMEM((N_DEV * S_LOC, 128), jnp.bfloat16),
            tile(N_DEV),
            tile(N_DEV),
            pltpu.SemaphoreType.DMA((5,)),
            pltpu.SemaphoreType.DMA((12,)),
            pltpu.SemaphoreType.DMA((12,)),
        ],
        compiler_params=pltpu.CompilerParams(
            collective_id=0, vmem_limit_bytes=64 * 1024 * 1024),
    )(x.reshape(ROWS, D), Wq, Wk, Wv, Wo)
    return out
```

```python
import numpy as np

import jax
import jax.numpy as jnp
from jax import lax
from jax.experimental import pallas as pl
from jax.experimental.pallas import tpu as pltpu

N_DEV = 4
B = 2
S_LOC = 128
ROWS = B * S_LOC
D = 512
H = 4
DH = 64
HD = H * DH
SCALE = 0.125

_MESH = pl.DeviceIdType.MESH
_C_V, _C_K, _C_Q, _C_C = 0, 1, 2, 3
_N_CLS = 4
_T_V, _T_K, _T_Q = 0, 1, 2
_ORDER = (2, 1, 3)


def _rope_tables(me):
    lane = lax.broadcasted_iota(jnp.int32, (8, 128), 1)
    fidx = (lane % DH) // 2
    inv_np = (1.0 / (10000.0 ** (np.arange(0, DH, 2) / DH))).astype(np.float32)
    inv = jnp.zeros((8, 128), jnp.float32)
    for i in range(DH // 2):
        inv = jnp.where(fidx == i, jnp.float32(inv_np[i]), inv)
    inv = jnp.broadcast_to(inv[0:1, :], (S_LOC, 128))
    row = lax.broadcasted_iota(jnp.int32, (S_LOC, 128), 0)
    pos = (row + me * S_LOC).astype(jnp.float32)
    ang = pos * inv
    lane2 = lax.broadcasted_iota(jnp.int32, (S_LOC, 128), 1)
    cos_t = jnp.cos(ang)
    sin_t = jnp.sin(ang)
    sin_t = jnp.where(lane2 % 2 == 0, -sin_t, sin_t)
    return cos_t, sin_t


def _rope(t, cos_t, sin_t):
    lane = lax.broadcasted_iota(jnp.int32, t.shape, 1)
    swapped = jnp.where(lane % 2 == 0, pltpu.roll(t, 127, 1), pltpu.roll(t, 1, 1))
    return t * cos_t + swapped * sin_t


def pallas_dist_rope_attn_qseq_b2_sq128_d512_hq4_dh64_kernel(
    x: jax.Array,
    Wq: jax.Array,
    Wk: jax.Array,
    Wv: jax.Array,
    Wo: jax.Array,
):
    def body(x_hbm, wq_hbm, wk_hbm, wv_hbm, wo_hbm, out_v,
             x_v, xb_v, w_v, wo_v, wo2,
             st, qq, kk, vv, sc, rc,
             ld_sems, ssem, rsem):
        me = lax.axis_index("i")
        w_hbm = (wv_hbm, wk_hbm, wq_hbm)
        j0 = 1 - me // 2

        def slot_of(h):
            return 2 * jnp.bitwise_xor(h // 2, j0) + h % 2

        x_load = pltpu.make_async_copy(x_hbm, x_v, ld_sems.at[0])
        w_loads = []
        for t in range(3):
            row = []
            for step in range(2):
                j = j0 if step == 0 else 1 - j0
                row.append(pltpu.make_async_copy(
                    w_hbm[t].at[:, pl.ds(pl.multiple_of(j * 128, 128), 128)],
                    w_v.at[t, step], ld_sems.at[1 + 2 * t + step]))
            w_loads.append(row)
        wo_load = pltpu.make_async_copy(wo_hbm, wo_v, ld_sems.at[7])
        x_load.start()
        for t, step in ((_T_Q, 0), (_T_K, 0), (_T_K, 1),
                        (_T_V, 0), (_T_V, 1), (_T_Q, 1)):
            w_loads[t][step].start()
        wo_load.start()

        bsem = pltpu.get_barrier_semaphore()
        for d in range(1, N_DEV):
            pl.semaphore_signal(bsem, inc=1, device_id=((me + d) % N_DEV,),
                                device_id_type=_MESH)

        cos_t, sin_t = _rope_tables(me)
        lo = lax.broadcasted_iota(jnp.int32, (S_LOC, 128), 1) < DH

        def src_of(d):
            return (me + N_DEV - d) % N_DEV

        def dst_of(d):
            return (me + d) % N_DEV

        def remote(cls, d, src_ref, dst_ref, dev):
            k = cls * 3 + (d - 1)
            return pltpu.make_async_remote_copy(
                src_ref=src_ref, dst_ref=dst_ref,
                send_sem=ssem.at[k], recv_sem=rsem.at[k],
                device_id=(dev,), device_id_type=_MESH)

        def rows_of(ref, idx):
            return ref.at[pl.ds(pl.multiple_of(idx * S_LOC, S_LOC), S_LOC), :]

        def project_pair(t, step):
            wb = w_v[t, step].astype(jnp.bfloat16)
            col = jnp.dot(xb_v[...], wb, preferred_element_type=jnp.float32)
            top, bot = col[0:S_LOC], col[S_LOC:ROWS]
            if t != _T_V:
                top = _rope(top, cos_t, sin_t)
                bot = _rope(bot, cos_t, sin_t)
            if t == _T_Q:
                top = top * SCALE
                bot = bot * SCALE
            even = jnp.where(lo, top, pltpu.roll(bot, DH, 1))
            odd = jnp.where(lo, pltpu.roll(top, DH, 1), bot)
            st[t, 2 * step] = even.astype(jnp.bfloat16)
            st[t, 2 * step + 1] = odd.astype(jnp.bfloat16)

        def ship_kv(t, step, e):
            cls, dst = (_C_V, vv) if t == _T_V else (_C_K, kk)
            j = j0 if step == 0 else 1 - j0
            h = 2 * j + e
            slot = 2 * step + e

            @pl.when(h != me)
            def _():
                d = (h + N_DEV - me) % N_DEV
                remote(cls, d, st.at[t, slot], rows_of(dst, me), h).start()

            @pl.when(h == me)
            def _():
                rows_of(dst, me)[...] = st[t, slot]

        def send_q(d):
            dev = dst_of(d)
            remote(_C_Q, d, st.at[_T_Q, slot_of(dev)], qq.at[me], dev).start()

        x_load.wait()
        xb_v[...] = x_v[...].astype(jnp.bfloat16)
        e0 = me % 2

        w_loads[_T_Q][0].wait()
        project_pair(_T_Q, 0)
        pl.semaphore_wait(bsem, N_DEV - 1)
        send_q(2)
        for t in (_T_K, _T_V):
            for step in range(2):
                w_loads[t][step].wait()
                project_pair(t, step)
                if step == 0:
                    ship_kv(t, step, e0)
                    ship_kv(t, step, 1 - e0)
                else:
                    ship_kv(t, step, 0)
                    ship_kv(t, step, 1)
        w_loads[_T_Q][1].wait()
        project_pair(_T_Q, 1)
        send_q(1)
        send_q(3)

        for d in _ORDER:
            remote(_C_V, d, st.at[_T_V, 0], rows_of(vv, src_of(d)), 0).wait_recv()
        for d in _ORDER:
            remote(_C_K, d, st.at[_T_K, 0], rows_of(kk, src_of(d)), 0).wait_recv()

        def attend(qp):
            qf = qp.astype(jnp.float32)
            lhs = jnp.concatenate(
                [jnp.where(lo, qf, 0.0), jnp.where(lo, 0.0, qf)], axis=0
            ).astype(jnp.bfloat16)
            s = lax.dot_general(lhs, kk[...], (((1,), (1,)), ((), ())),
                                preferred_element_type=jnp.float32)
            m = jnp.max(s, axis=1, keepdims=True)
            p = jnp.exp(s - m)
            l = jnp.sum(p, axis=1, keepdims=True)
            c = jnp.dot(p.astype(jnp.bfloat16), vv[...],
                        preferred_element_type=jnp.float32)
            c = c * (1.0 / l)
            return jnp.where(lo, c[0:S_LOC], c[S_LOC:ROWS]).astype(jnp.bfloat16)

        for d in _ORDER:
            src = src_of(d)
            remote(_C_Q, d, st.at[_T_Q, 0], qq.at[src], src).wait_recv()
            sc[src] = attend(qq[src])
            remote(_C_C, N_DEV - d, sc.at[src], rc.at[me], src).start()

        wo_load.wait()
        for h in range(H):
            blk = wo_v[h * DH:(h + 1) * DH, :].astype(jnp.bfloat16)
            wo2[h, 0:DH, :] = blk
            wo2[h, DH:2 * DH, :] = blk
        rc[me] = attend(st[_T_Q, slot_of(me)])

        def head_out(h):
            tf = rc[h].astype(jnp.float32)
            lhs = jnp.concatenate(
                [jnp.where(lo, tf, 0.0), jnp.where(lo, 0.0, tf)], axis=0
            ).astype(jnp.bfloat16)
            return jnp.dot(lhs, wo2[h], preferred_element_type=jnp.float32)

        res = head_out(me)
        for b in range(B):
            out_v[b] = res[b * S_LOC:(b + 1) * S_LOC]
        for d in (2, 3, 1):
            src = src_of(d)
            remote(_C_C, d, sc.at[0], rc.at[src], src).wait_recv()
            res = head_out(src)
            for b in range(B):
                out_v[b] = out_v[b] + res[b * S_LOC:(b + 1) * S_LOC]

        for d in range(1, N_DEV):
            remote(_C_V, d, st.at[_T_V, 0], rows_of(vv, me), 0).wait_send()
            remote(_C_K, d, st.at[_T_K, 0], rows_of(kk, me), 0).wait_send()
            remote(_C_Q, d, st.at[_T_Q, 0], qq.at[me], 0).wait_send()
            remote(_C_C, d, sc.at[0], rc.at[me], 0).wait_send()

    hbm = pl.BlockSpec(memory_space=pltpu.HBM)
    return pl.pallas_call(
        body,
        out_shape=jax.ShapeDtypeStruct((B, S_LOC, D), jnp.float32),
        in_specs=[hbm] * 5,
        out_specs=pl.BlockSpec(memory_space=pltpu.VMEM),
        scratch_shapes=[
            pltpu.VMEM((ROWS, D), jnp.float32),
            pltpu.VMEM((ROWS, D), jnp.bfloat16),
            pltpu.VMEM((3, 2, D, 128), jnp.float32),
            pltpu.VMEM((HD, D), jnp.float32),
            pltpu.VMEM((H, 2 * DH, D), jnp.bfloat16),
            pltpu.VMEM((3, H, S_LOC, 128), jnp.bfloat16),
            pltpu.VMEM((N_DEV, S_LOC, 128), jnp.bfloat16),
            pltpu.VMEM((N_DEV * S_LOC, 128), jnp.bfloat16),
            pltpu.VMEM((N_DEV * S_LOC, 128), jnp.bfloat16),
            pltpu.VMEM((N_DEV, S_LOC, 128), jnp.bfloat16),
            pltpu.VMEM((N_DEV, S_LOC, 128), jnp.bfloat16),
            pltpu.SemaphoreType.DMA((8,)),
            pltpu.SemaphoreType.DMA((_N_CLS * 3,)),
            pltpu.SemaphoreType.DMA((_N_CLS * 3,)),
        ],
        compiler_params=pltpu.CompilerParams(
            collective_id=0, vmem_limit_bytes=64 * 1024 * 1024),
    )(x.reshape(ROWS, D), Wq, Wk, Wv, Wo)
```
